```python
import numpy as np

kernel_name = "dist_ar_i_i_m2048_n512"

def setup_inputs():
    return {"x": np.random.randn(8192, 512).astype(np.float32)}

def reference(x: np.ndarray) -> np.ndarray:
    return x.reshape(4, 2048, 512).sum(axis=0)
```

```python
import jax
import jax.numpy as jnp
import numpy as np
from jax import lax
from jax.experimental import pallas as pl
from jax.experimental.pallas import tpu as pltpu

I32, BF16, F32 = jnp.int32, jnp.bfloat16, jnp.float32
ROWS, COLS = 2048, 512
PIECE = ROWS // 4
SET_ROWS = 64
SETS = 4
MSG_ROWS = SETS * SET_ROWS

SIGN, MAG, BYTE = np.array([0x80008000, 0x7FFF7FFF, 0x00FF00FF], np.uint32).view(np.int32)

SET_WORDS = 9
OWN, POOLED = 6, 3
STREAM = OWN + POOLED
W_HEAD = SETS * SET_WORDS
W_OWN = W_HEAD + 1
W_POOL = W_OWN + OWN
W_END = W_OWN + 8 * SETS + 2
TOP_DROP, UNCODED = 8, 63
FITS, TWO_POOLS, OVERFLOWS = 0, 1, 2

P_LEN, P_LONG, P_TOP = STREAM, STREAM + 1, STREAM + 2

DETOUR = 8
DIRECT = 16 - DETOUR
DIRECT_ROWS = 16 * pl.cdiv(DIRECT, 4)
DIRECT_WORDS = 1 + pl.cdiv(DIRECT, 2)
ODD_ORDER = ((0, 0), (0, 1), (0, 2), (1, 0), (0, 3), (1, 1), (1, 2), (1, 3))
EVEN_ORDER = ((0, 0), (1, 0), (0, 1), (1, 1), (0, 2), (1, 2), (0, 3), (1, 3))
TAIL = 1


def _span(start, size, align):
    if not isinstance(start, int):
        start = pl.multiple_of(start, align)
    return pl.ds(start, size)


def _word(i):
    return _span(8 * i, 8, 8)


def _tile(row, j):
    return _span(row + 16 * (j // 4), 16, 16), pl.ds(128 * (j % 4), 128)


def _srl(v, n):
    return lax.shift_right_logical(v, np.int32(n) if isinstance(n, int) else n)


def _roll(v, k):
    return pltpu.roll(v, k, 0) if k else v


def _zeros():
    return jnp.zeros((8, 128), I32)


def _sublane():
    return lax.broadcasted_iota(I32, (8, 128), 0)


def _loop(lo, hi, f):
    lax.fori_loop(lo, hi, lambda i, _: f(i), None)


def _top(code):
    top = (code + 1) << 4
    return top | (top << 16)


def _flip(top, v):
    nonzero = (v + MAG) & SIGN
    return (top - v) & (nonzero - _srl(nonzero, 15))


def _pool_layout(head):
    n = _srl(head, 26)
    end = n
    for k in (1, 2, 4):
        end = end + jnp.where(_sublane() >= k, _roll(end, k), 0)
    form = jnp.where(end > 128, float(TWO_POOLS), float(FITS))
    form = jnp.where((n == UNCODED) | (end > 256), float(OVERFLOWS), form)
    start = 2 * (end - n)
    return jnp.max(form).astype(I32), start >> 5, start & 31


def _pack_begin(state):
    for i in range(P_TOP + 1):
        state[i] = _zeros()


def _pack_low(words, s, msg, state):
    mags = [w & MAG for w in words]
    peak = [lax.bitcast_convert_type(v, F32) for v in mags + [m << 16 for m in mags]]
    while len(peak) > 1:
        peak = [jnp.maximum(a, b) for a, b in zip(peak[0::2], peak[1::2])]
    code = jnp.maximum(lax.bitcast_convert_type(peak[0], I32) >> 20, 7)
    code = jnp.where(peak[0] != peak[0], 2047, code)
    code = jnp.maximum(code, state[P_TOP + s] - TOP_DROP)
    state[P_TOP + s + 1] = code
    top = _top(code)
    us = [_flip(top, m) for m in mags]
    signs = _zeros()
    for j, w in enumerate(words):
        signs = signs | _srl(w & SIGN, j)
    msg[_word(s * SET_WORDS)] = signs
    for i in range(8):
        msg[_word(s * SET_WORDS + 1 + i)] = (us[2 * i] & BYTE) | ((us[2 * i + 1] & BYTE) << 8)
    return us


def _pack_high(us, state):
    stream = [state[i] for i in range(STREAM)]
    length, longest = state[P_LEN], state[P_LONG]
    for g in range(4):
        bits, total = _zeros(), _zeros()
        for k in range(8):
            u = us[4 * g + k // 2]
            total = total + (u >> 24 if k % 2 else (u >> 8) & 0xFF)
            bits = bits | ((1 << k) << (total & 31))
        lo, hi = bits << (length & 31), _srl(_srl(bits, 1), 31 - (length & 31))
        here = [length >> 5 == i for i in range(STREAM)]
        stream = [
            v | jnp.where(here[i], lo, jnp.where(here[i - 1], hi, 0) if i else 0)
            for i, v in enumerate(stream)
        ]
        length, longest = length + total + 8, jnp.maximum(longest, total)
    for i, v in enumerate(stream + [length, longest]):
        state[i] = v


def _pack_end(msg, state, tile_of):
    codes = [state[P_TOP + 1 + s] for s in range(SETS)]
    head = codes[0]
    unfit = (state[P_LONG] > 24) | (state[P_LEN] > 32 * STREAM)
    for s in range(1, SETS):
        step = codes[s] - codes[s - 1] + TOP_DROP
        head, unfit = head | ((step & 31) << (6 + 5 * s)), unfit | (step > 31)
    pooled = (jnp.maximum(state[P_LEN] - 32 * OWN, 0) + 1) >> 1
    head = head | (jnp.where(unfit, UNCODED, pooled) << 26)
    msg[_word(W_HEAD)] = head
    for i in range(OWN):
        msg[_word(W_OWN + i)] = state[i]
    form, first, bit = _pool_layout(head)
    rest = [state[OWN + i] for i in range(POOLED)]
    moved = [
        (rest[i] << bit if i < POOLED else 0) | (_srl(_srl(rest[i - 1], 1), 31 - bit) if i else 0)
        for i in range(POOLED + 1)
    ]
    for p in range(2):
        pool = _zeros()
        for k in range(8):
            which, part = ((_sublane() + k) & 7) + 8 * p - first, 0
            for i, v in enumerate(moved):
                part = jnp.where(which == i, v, part)
            pool = pool | _roll(part, k)
        msg[_word(W_POOL + p)] = pool

    @pl.when(form == OVERFLOWS)
    def _():
        def high_bytes(s):
            top = _top(state[P_TOP + 1 + s])
            for i in range(8):
                a, b = (pltpu.bitcast(tile_of(s, j), I32) & MAG for j in (2 * i, 2 * i + 1))
                a, b = _flip(top, a) & ~BYTE, _flip(top, b) & ~BYTE
                msg[_word(W_OWN + 8 * s + i)] = _srl(a, 8) | b

        _loop(0, SETS, high_bytes)
        for i in range(2):
            msg[_word(W_END - 2 + i)] = codes[2 * i] | (codes[2 * i + 1] << 16)

    return form


def _unpack_begin(msg, state, wait_pool, wait_rest):
    head = msg[_word(W_HEAD)]
    form, first, bit = _pool_layout(head)

    @pl.when(form == FITS)
    def _():
        msg[_word(W_POOL + 1)] = _zeros()

    pl.when(form == TWO_POOLS)(wait_pool)

    @pl.when(form != OVERFLOWS)
    def _():
        code = head & 2047
        for s in range(SETS):
            if s:
                code = code + ((head >> (6 + 5 * s)) & 31) - TOP_DROP
            state[STREAM + s] = _top(code)
        moved = [_zeros()] * (POOLED + 1)
        for p in range(2):
            pool = msg[_word(W_POOL + p)]
            for k in range(8):
                which = ((_sublane() + k) & 7) + 8 * p - first
                part = _roll(pool, (8 - k) % 8)
                moved = [jnp.where(which == i, part, v) for i, v in enumerate(moved)]
        for i in range(OWN):
            state[i] = msg[_word(W_OWN + i)]
        for i in range(POOLED):
            state[OWN + i] = _srl(moved[i], bit) | ((moved[i + 1] << 1) << (31 - bit))

    @pl.when(form == OVERFLOWS)
    def _():
        wait_rest()
        for s in range(SETS):
            codes = msg[_word(W_END - 2 + s // 2)]
            state[STREAM + s] = _top(_srl(codes, 16 * (s % 2)) & 0xFFFF)

    return form == OVERFLOWS


def _unpack_high(s, msg, state, uncoded):
    if uncoded:
        pairs = [msg[_word(W_OWN + 8 * s + i)] for i in range(8)]
        return [(pairs[j // 2] if j % 2 else pairs[j // 2] << 8) & ~BYTE for j in range(16)]
    stream, highs = [state[i] for i in range(STREAM)], []
    for _ in range(4):
        bits, above = stream[0], [32]
        for _ in range(8):
            above.append(lax.clz(bits ^ (bits - 1)))
            bits = bits & (bits - 1)
        gaps = [a - b for a, b in zip(above, above[1:])]
        highs += [((gaps[k] << 8) | (gaps[k + 1] << 24)) - 0x01000100 for k in (0, 2, 4, 6)]
        stream = [
            _srl(_srl(v, 1), 31 - above[8]) | (stream[i + 1] << above[8] if i + 1 < STREAM else 0)
            for i, v in enumerate(stream)
        ]
    for i, v in enumerate(stream):
        state[i] = v
    return highs


def _unpack_set(s, msg, state, high, pairs=range(8)):
    top, signs, tiles = state[STREAM + s], msg[_word(s * SET_WORDS)], {}
    for i in pairs:
        lows = msg[_word(s * SET_WORDS + 1 + i)]
        for j in (2 * i, 2 * i + 1):
            u = high(j) | ((_srl(lows, 8) if j % 2 else lows) & BYTE)
            tiles[j] = pltpu.bitcast(_flip(top, u) | ((signs << j) & SIGN), BF16)
    return tiles


def _all_reduce(
    x_hbm, out, given, kept, pair_sum, outbox, inbox, detour_out, detour_in, packer, unpacker,
    held, forms, given_sem, kept_sem, send_sem, recv_sem, detour_sem, entered_sem,
):
    me = lax.axis_index("i")
    odd = (me & 1) == 1
    lead = (me + 1) >> 2

    def peer(half):
        return jnp.where(half == 0, me ^ 1, 3 - me)

    def side(half):
        return jnp.where(half == 0, (me ^ (me >> 1)) & 1, me >> 1)

    def keep(half):
        return (2 * half + side(half)) * PIECE

    def give(half):
        return (2 * half + 1 - side(half)) * PIECE

    def rows(c, s, source):
        if c:
            return MSG_ROWS + SET_ROWS * s
        return SET_ROWS * ((s + (source == 2).astype(I32)) & 3)

    def each_link(f):
        _loop(0, 2, lambda link: f(link ^ lead))

    def signal(sem, chips):
        for chip in chips:
            pl.semaphore_signal(sem, inc=1, device_id=(chip,), device_id_type=pl.DeviceIdType.MESH)

    def remote(src, dst, send, recv, chip):
        return pltpu.make_async_remote_copy(
            src, dst, send, recv, device_id=(chip,), device_id_type=pl.DeviceIdType.MESH
        )

    def load_given(half, slot, start, size):
        return pltpu.make_async_copy(
            x_hbm.at[_span(give(half) + start, size, 16)],
            given.at[_span(half * PIECE + start, size, 16)],
            given_sem.at[7 * half + slot],
        )

    def load_set(half, s):
        return load_given(half, s, rows(0, s, me), SET_ROWS)

    def load_direct():
        return load_given(lead, 0, 0, DIRECT_ROWS)

    def load_detour():
        return load_given(lead, 4, DIRECT_ROWS, SET_ROWS - DIRECT_ROWS)

    def load_second(half, part):
        size = MSG_ROWS - SET_ROWS if part else SET_ROWS
        return load_given(half, 5 + part, MSG_ROWS + SET_ROWS * part, size)

    def load_kept(half, c):
        return pltpu.make_async_copy(
            x_hbm.at[_span(keep(half) + c * MSG_ROWS, MSG_ROWS, 16)],
            kept.at[_span(half * PIECE + c * MSG_ROWS, MSG_ROWS, 16)],
            kept_sem.at[2 * half + c],
        )

    def box(step, c, half):
        return 4 * step + 2 * c + half

    def copy(step, c, half, slot, start, size):
        i, words = box(step, c, half), _span(8 * start, 8 * size, 8)
        return remote(
            outbox.at[i, words], inbox.at[i, words], send_sem.at[8 * i + slot],
            recv_sem.at[8 * i + slot], peer(1 - half if step == 1 else half),
        )

    def copy_set(step, c, half, s, size=SET_WORDS):
        return copy(step, c, half, s, s * SET_WORDS, size)

    def copy_head(step, c, half):
        return copy(step, c, half, 4, W_HEAD, W_POOL + 1 - W_HEAD)

    def copy_pool(step, c, half):
        return copy(step, c, half, 5, W_POOL + 1, 1)

    def copy_rest(step, c, half):
        return copy(step, c, half, 6, W_POOL + 1, W_END - W_POOL - 1)

    def copy_last(half):
        return copy_set(2, 1, half, SETS - 1, SET_WORDS - TAIL)

    def copy_tail(half):
        return copy(2, 1, half, 7, W_HEAD - TAIL, TAIL)

    def copy_detour(half):
        return remote(detour_out, detour_in.at[half], detour_sem.at[2], detour_sem.at[half], 2)

    def finish(step, c, half, tile_of):
        form = _pack_end(outbox.at[box(step, c, half)], packer.at[half], tile_of)
        copy_head(step, c, half).start()
        pl.when(form == TWO_POOLS)(lambda: copy_pool(step, c, half).start())
        pl.when(form == OVERFLOWS)(lambda: copy_rest(step, c, half).start())
        if (step, c) == (2, 1):
            for s in range(1, SETS - 1):
                copy_set(step, c, half, s).start()
            copy_last(half).start()
            copy_tail(half).start()
        elif (step, c) != (0, 0):
            for s in range(1, SETS):
                copy_set(step, c, half, s).start()
        forms[box(step, c, half)] = form

    def receive(step, c, half, each_set):
        copy_head(step, c, half).wait_recv()
        msg, state = inbox.at[box(step, c, half)], unpacker.at[half]
        uncoded = _unpack_begin(
            msg, state,
            lambda: copy_pool(step, c, half).wait_recv(),
            lambda: copy_rest(step, c, half).wait_recv(),
        )
        for form, taken in ((False, jnp.logical_not(uncoded)), (True, uncoded)):
            pl.when(taken)(
                lambda: _loop(0, SETS, lambda s: each_set(s, lambda: _unpack_high(s, msg, state, form)))
            )

    def given_tile(half, c, s, j):
        return given[_tile(half * PIECE + rows(c, s, me), j)].astype(BF16)

    def pack_given(half, c, s, tiles=16):
        words = [pltpu.bitcast(given_tile(half, c, s, j), I32) for j in range(tiles)]
        words += [_zeros()] * (16 - tiles)
        return _pack_low(words, s, outbox.at[box(0, c, half)], packer.at[half])

    def hold(half, s, words):
        for j, w in enumerate(words):
            held[half, 16 * s + j] = w

    barrier = pltpu.get_barrier_semaphore()

    @pl.when(odd)
    def _():
        load_direct().start()
        signal(barrier, (2, 0))
        for t, (link, s) in enumerate(ODD_ORDER[1:]):
            load_set(link ^ lead, s).start()
            if t == 0:
                load_detour().start()
        for half in range(2):
            _pack_begin(packer.at[half])
        pl.semaphore_wait(barrier, 1)
        load_direct().wait()
        us = pack_given(lead, 0, 0, DIRECT)
        copy_set(0, 0, lead, 0, DIRECT_WORDS).start()
        hold(lead, 0, us)

    @pl.when(jnp.logical_not(odd))
    def _():
        for half, s in EVEN_ORDER[:2]:
            load_set(half, s).start()

        @pl.when(me == 2)
        def _():
            pl.semaphore_wait(barrier, 2)
            signal(entered_sem, (1, 3))

        @pl.when(me == 0)
        def _():
            signal(barrier, (1, 3))
            for half in range(2):
                for i in range(DIRECT_WORDS, SET_WORDS):
                    inbox[box(0, 0, half), _word(i)] = _zeros()

        for half, s in EVEN_ORDER[2:]:
            load_set(half, s).start()
        for half in range(2):
            _pack_begin(packer.at[half])

    def first_sets(t):
        odd_order, even_order = (
            sum((4 * link + s) << (3 * i) for i, (link, s) in enumerate(order))
            for order in (ODD_ORDER, EVEN_ORDER)
        )
        entry = jnp.where(odd, odd_order, even_order) >> (3 * t)
        half, s = ((entry >> 2) & 1) ^ lead, entry & 3
        load_set(half, s).wait()

        @pl.when((me == 2) & (s == SETS - 1))
        def _():
            copy_detour(half).wait_recv()
            for i in range(DETOUR):
                at = _tile(half * PIECE, DIRECT + i)
                given[at] = given[at] + pltpu.bitcast(detour_in[half, _word(i)], BF16).astype(F32)

        us = pack_given(half, 0, s)

        @pl.when(odd & (t == 2))
        def _():
            load_detour().wait()
            for i in range(DETOUR):
                at = _tile(lead * PIECE, DIRECT + i)
                detour_out[_word(i)] = pltpu.bitcast(given[at].astype(BF16), I32)
                given[at] = jnp.zeros((16, 128), F32)
            pl.semaphore_wait(entered_sem, 1)
            copy_detour(lead).start()

        @pl.when((me == 0) & (t == 1))
        def _():
            pl.semaphore_wait(barrier, 2)
            copy_set(0, 0, lead, 0).start()

        pl.when((me != 0) | (t != 0))(lambda: copy_set(0, 0, half, s).start())
        hold(half, s, us)

        @pl.when(t == 3)
        def _():
            for link in range(2):
                for part in range(2):
                    load_second(link ^ lead, part).start()

    _loop(me & 1, 2 * SETS, first_sets)
    for link in range(2):
        load_kept(link ^ lead, 0).start()

    @each_link
    def _(half):
        _loop(
            0, SETS,
            lambda s: _pack_high([held[half, 16 * s + j] for j in range(16)], packer.at[half]),
        )
        finish(0, 0, half, lambda s, j: given_tile(half, 0, s, j))

    @each_link
    def _(half):
        def each_set(s):
            pl.when(s == 0)(lambda: load_second(half, 0).wait())
            pl.when(s == 1)(lambda: load_second(half, 1).wait())
            _pack_high(pack_given(half, 1, s), packer.at[half])
            pl.when(s == 0)(lambda: copy_set(0, 1, half, 0).start())

        _pack_begin(packer.at[half])
        _loop(0, SETS, each_set)
        finish(0, 1, half, lambda s, j: given_tile(half, 1, s, j))

    for link in range(2):
        load_kept(link ^ lead, 1).start()

    def add_and_send(step, c, half):
        msg, state = inbox.at[box(step - 1, c, half)], unpacker.at[half]
        own = kept if step == 1 else pair_sum
        sums, base = (pair_sum, half * PIECE) if step == 1 else (out, keep(half))
        source = peer(half) if step == 1 else me ^ 2
        if step == 1:
            load_kept(half, c).wait()
        if (step, c) == (1, 0):
            pl.when(me == 0)(lambda: copy_set(0, 0, half, 0, DIRECT_WORDS).wait_recv())
            pl.when(me != 0)(lambda: copy_set(0, 0, half, 0).wait_recv())
            for s in range(1, SETS):
                copy_set(0, 0, half, s).wait_recv()

        def sum_tile(s, j):
            return sums[_tile(base + rows(c, s, source), j)]

        def each_set(s, unpack_high):
            if (step, c) != (1, 0):
                copy_set(step - 1, c, half, s).wait_recv()
            highs, row = unpack_high(), rows(c, s, source)
            for j, theirs in _unpack_set(s, msg, state, lambda j: highs[j]).items():
                mine = own[_tile(half * PIECE + row, j)].astype(F32)
                sums[_tile(base + row, j)] = (mine + theirs.astype(F32)).astype(BF16)
            words = [pltpu.bitcast(sum_tile(s, j), I32) for j in range(16)]
            us = _pack_low(words, s, outbox.at[box(step, c, half)], packer.at[half])
            _pack_high(us, packer.at[half])
            pl.when(s == 0)(lambda: copy_set(step, c, half, 0).start())

        _pack_begin(packer.at[half])
        receive(step - 1, c, half, each_set)
        finish(step, c, half, sum_tile)

    for step in (1, 2):
        for c in range(2):
            each_link(lambda half: add_and_send(step, c, half))

    def wait_sent(step, c, sets=SETS):
        for half in range(2):
            if (step, c) == (0, 0):
                short = odd & (lead == half)
                pl.when(short)(lambda: copy_set(0, 0, half, 0, DIRECT_WORDS).wait_send())
                pl.when(jnp.logical_not(short))(lambda: copy_set(0, 0, half, 0).wait_send())
            for s in range(int((step, c) == (0, 0)), sets):
                copy_set(step, c, half, s).wait_send()
            copy_head(step, c, half).wait_send()
            form = forms[box(step, c, half)]
            pl.when(form == TWO_POOLS)(lambda: copy_pool(step, c, half).wait_send())
            pl.when(form == OVERFLOWS)(lambda: copy_rest(step, c, half).wait_send())

    pl.when(odd)(lambda: copy_detour(lead).wait_send())
    for step in range(2):
        for c in range(2):
            wait_sent(step, c)

    def store(c, half, s, pairs=range(8)):
        msg, state = inbox.at[box(2, c, half)], unpacker.at[half]
        tiles = _unpack_set(s, msg, state, lambda j: held[half, 16 * s + j], pairs)
        for j, tile in tiles.items():
            out[_tile(give(half) + rows(c, s, peer(half) ^ 2), j)] = tile

    for c in range(2):
        each_link(lambda half: receive(2, c, half, lambda s, high: hold(half, s, high())))

        def early_set(t):
            s, half = t >> 1, (t & 1) ^ lead
            copy_set(2, c, half, s).wait_recv()
            store(c, half, s)

        _loop(0, 2 * (SETS - c), early_set)
        wait_sent(2, c, SETS - c)

    @each_link
    def _(half):
        copy_last(half).wait_recv()
        store(1, half, SETS - 1, range(8 - TAIL))

    for half in range(2):
        copy_last(half).wait_send()
        copy_tail(half).wait_send()
    for link in range(2):
        copy_tail(link ^ lead).wait_recv()
        store(1, link ^ lead, SETS - 1, range(8 - TAIL, 8))


def pallas_dist_ar_i_i_m2048_n512_kernel(x: jax.Array):
    assert x.shape == (ROWS, COLS) and x.dtype == F32
    dma = pltpu.SemaphoreType.DMA
    messages = 3 * 2 * 2
    return pl.pallas_call(
        _all_reduce,
        out_shape=jax.ShapeDtypeStruct((ROWS, COLS), BF16),
        in_specs=[pl.BlockSpec(memory_space=pl.ANY)],
        out_specs=pl.BlockSpec(memory_space=pltpu.VMEM),
        scratch_shapes=[
            pltpu.VMEM((2 * PIECE, COLS), F32),
            pltpu.VMEM((2 * PIECE, COLS), F32),
            pltpu.VMEM((2 * PIECE, COLS), BF16),
            pltpu.VMEM((messages, 8 * W_END, 128), I32),
            pltpu.VMEM((messages, 8 * W_END, 128), I32),
            pltpu.VMEM((8 * DETOUR, 128), I32),
            pltpu.VMEM((2, 8 * DETOUR, 128), I32),
            pltpu.VMEM((2, P_TOP + 1 + SETS, 8, 128), I32),
            pltpu.VMEM((2, STREAM + SETS, 8, 128), I32),
            pltpu.VMEM((2, 16 * SETS, 8, 128), I32),
            pltpu.SMEM((messages,), I32),
            dma((14,)),
            dma((4,)),
            dma((8 * messages,)),
            dma((8 * messages,)),
            dma((3,)),
            pltpu.SemaphoreType.REGULAR,
        ],
        compiler_params=pltpu.CompilerParams(
            collective_id=0,
            vmem_limit_bytes=32 * 2**20,
            disable_semaphore_checks=True,
        ),
    )(x)
```

```python
import jax
import jax.numpy as jnp
import numpy as np
from jax import lax
from jax.experimental import pallas as pl
from jax.experimental.pallas import tpu as pltpu

I32, BF16, F32 = jnp.int32, jnp.bfloat16, jnp.float32
ROWS, COLS = 2048, 512
PIECE = ROWS // 4
SET_ROWS = 64
SETS = 4
MSG_ROWS = SETS * SET_ROWS

SIGN, MAG, BYTE = np.array([0x80008000, 0x7FFF7FFF, 0x00FF00FF], np.uint32).view(np.int32)

SET_WORDS = 9
OWN, POOLED = 6, 3
STREAM = OWN + POOLED
W_HEAD = SETS * SET_WORDS
W_OWN = W_HEAD + 1
W_POOL = W_OWN + OWN
W_END = W_OWN + 8 * SETS + 2
TOP_DROP, UNCODED = 8, 63
FITS, TWO_POOLS, OVERFLOWS = 0, 1, 2
GROUPS = (7, 7, 6, 6, 6)

P_LEN, P_LONG, P_TOP = STREAM, STREAM + 1, STREAM + 2

DETOUR = 8
DIRECT = 16 - DETOUR
DIRECT_ROWS = 16 * pl.cdiv(DIRECT, 4)
DIRECT_WORDS = 1 + pl.cdiv(DIRECT, 2)
ODD_ORDER = ((0, 0), (0, 1), (0, 2), (1, 0), (0, 3), (1, 1), (1, 2), (1, 3))
EVEN_ORDER = ((0, 0), (1, 0), (0, 1), (1, 1), (0, 2), (1, 2), (0, 3), (1, 3))
TAIL = 1


def _span(start, size, align):
    if not isinstance(start, int):
        start = pl.multiple_of(start, align)
    return pl.ds(start, size)


def _word(i):
    return _span(8 * i, 8, 8)


def _tile(row, j):
    return _span(row + 16 * (j // 4), 16, 16), pl.ds(128 * (j % 4), 128)


def _srl(v, n):
    return lax.shift_right_logical(v, np.int32(n) if isinstance(n, int) else n)


def _roll(v, k):
    return pltpu.roll(v, k, 0) if k else v


def _zeros():
    return jnp.zeros((8, 128), I32)


def _sublane():
    return lax.broadcasted_iota(I32, (8, 128), 0)


def _loop(lo, hi, f):
    lax.fori_loop(lo, hi, lambda i, _: f(i), None)


def _top(code):
    top = (code + 1) << 4
    return top | (top << 16)


def _flip(top, v):
    nonzero = (v + MAG) & SIGN
    return (top - v) & (nonzero - _srl(nonzero, 15))


def _pool_layout(head):
    n = _srl(head, 26)
    end = n
    for k in (1, 2, 4):
        end = end + jnp.where(_sublane() >= k, _roll(end, k), 0)
    form = jnp.where(end > 128, float(TWO_POOLS), float(FITS))
    form = jnp.where((n == UNCODED) | (end > 256), float(OVERFLOWS), form)
    start = 2 * (end - n)
    return jnp.max(form).astype(I32), start >> 5, start & 31


def _pack_begin(state):
    for i in range(P_TOP + 1):
        state[i] = _zeros()


def _pack_low(words, s, msg, state):
    mags = [w & MAG for w in words]
    peak = [lax.bitcast_convert_type(v, F32) for v in mags + [m << 16 for m in mags]]
    while len(peak) > 1:
        peak = [jnp.maximum(a, b) for a, b in zip(peak[0::2], peak[1::2])]
    code = jnp.maximum(lax.bitcast_convert_type(peak[0], I32) >> 20, 7)
    code = jnp.where(peak[0] != peak[0], 2047, code)
    code = jnp.maximum(code, state[P_TOP + s] - TOP_DROP)
    state[P_TOP + s + 1] = code
    top = _top(code)
    us = [_flip(top, m) for m in mags]
    signs = _zeros()
    for j, w in enumerate(words):
        signs = signs | _srl(w & SIGN, j)
    msg[_word(s * SET_WORDS)] = signs
    for i in range(8):
        msg[_word(s * SET_WORDS + 1 + i)] = (us[2 * i] & BYTE) | ((us[2 * i + 1] & BYTE) << 8)
    return us


def _pack_high(us, state):
    stream = [state[i] for i in range(STREAM)]
    length, longest = state[P_LEN], state[P_LONG]
    highs = iter([high for u in us for high in ((u >> 8) & 0xFF, u >> 24)])
    for group in GROUPS:
        bits, total = _zeros(), _zeros()
        for k in range(group):
            total = total + next(highs)
            bits = bits | ((1 << k) << (total & 31))
        total = total + group
        lo, hi = bits << (length & 31), _srl(_srl(bits, 1), 31 - (length & 31))
        here = [length >> 5 == i for i in range(STREAM)]
        stream = [
            v | jnp.where(here[i], lo, jnp.where(here[i - 1], hi, 0) if i else 0)
            for i, v in enumerate(stream)
        ]
        length, longest = length + total, jnp.maximum(longest, total)
    for i, v in enumerate(stream + [length, longest]):
        state[i] = v


def _pack_end(msg, state, tile_of):
    codes = [state[P_TOP + 1 + s] for s in range(SETS)]
    head = codes[0]
    unfit = (state[P_LONG] > 32) | (state[P_LEN] > 32 * STREAM)
    for s in range(1, SETS):
        step = codes[s] - codes[s - 1] + TOP_DROP
        head, unfit = head | ((step & 31) << (6 + 5 * s)), unfit | (step > 31)
    pooled = (jnp.maximum(state[P_LEN] - 32 * OWN, 0) + 1) >> 1
    head = head | (jnp.where(unfit, UNCODED, pooled) << 26)
    msg[_word(W_HEAD)] = head
    for i in range(OWN):
        msg[_word(W_OWN + i)] = state[i]
    form, first, bit = _pool_layout(head)
    rest = [state[OWN + i] for i in range(POOLED)]
    moved = [
        (rest[i] << bit if i < POOLED else 0) | (_srl(_srl(rest[i - 1], 1), 31 - bit) if i else 0)
        for i in range(POOLED + 1)
    ]
    for p in range(2):
        pool = _zeros()
        for k in range(8):
            which, part = ((_sublane() + k) & 7) + 8 * p - first, 0
            for i, v in enumerate(moved):
                part = jnp.where(which == i, v, part)
            pool = pool | _roll(part, k)
        msg[_word(W_POOL + p)] = pool

    @pl.when(form == OVERFLOWS)
    def _():
        def high_bytes(s):
            top = _top(state[P_TOP + 1 + s])
            for i in range(8):
                a, b = (pltpu.bitcast(tile_of(s, j), I32) & MAG for j in (2 * i, 2 * i + 1))
                a, b = _flip(top, a) & ~BYTE, _flip(top, b) & ~BYTE
                msg[_word(W_OWN + 8 * s + i)] = _srl(a, 8) | b

        _loop(0, SETS, high_bytes)
        for i in range(2):
            msg[_word(W_END - 2 + i)] = codes[2 * i] | (codes[2 * i + 1] << 16)

    return form


def _unpack_begin(msg, state, wait_pool, wait_rest):
    head = msg[_word(W_HEAD)]
    form, first, bit = _pool_layout(head)

    @pl.when(form == FITS)
    def _():
        msg[_word(W_POOL + 1)] = _zeros()

    pl.when(form == TWO_POOLS)(wait_pool)

    @pl.when(form != OVERFLOWS)
    def _():
        code = head & 2047
        for s in range(SETS):
            if s:
                code = code + ((head >> (6 + 5 * s)) & 31) - TOP_DROP
            state[STREAM + s] = _top(code)
        moved = [_zeros()] * (POOLED + 1)
        for p in range(2):
            pool = msg[_word(W_POOL + p)]
            for k in range(8):
                which = ((_sublane() + k) & 7) + 8 * p - first
                part = _roll(pool, (8 - k) % 8)
                moved = [jnp.where(which == i, part, v) for i, v in enumerate(moved)]
        for i in range(OWN):
            state[i] = msg[_word(W_OWN + i)]
        for i in range(POOLED):
            state[OWN + i] = _srl(moved[i], bit) | ((moved[i + 1] << 1) << (31 - bit))

    @pl.when(form == OVERFLOWS)
    def _():
        wait_rest()
        for s in range(SETS):
            codes = msg[_word(W_END - 2 + s // 2)]
            state[STREAM + s] = _top(_srl(codes, 16 * (s % 2)) & 0xFFFF)

    return form == OVERFLOWS


def _unpack_high(s, msg, state, uncoded):
    if uncoded:
        pairs = [msg[_word(W_OWN + 8 * s + i)] for i in range(8)]
        return [(pairs[j // 2] if j % 2 else pairs[j // 2] << 8) & ~BYTE for j in range(16)]
    stream, sizes = [state[i] for i in range(STREAM)], []
    for group in GROUPS:
        bits, above = stream[0], 32
        for _ in range(group):
            before, above = above, lax.clz(bits ^ (bits - 1))
            bits = bits & (bits - 1)
            sizes.append(before - above)
        stream = [
            _srl(_srl(v, 1), 31 - above) | (stream[i + 1] << above if i + 1 < STREAM else 0)
            for i, v in enumerate(stream)
        ]
    for i, v in enumerate(stream):
        state[i] = v
    return [((a << 8) | (b << 24)) - 0x01000100 for a, b in zip(sizes[0::2], sizes[1::2])]


def _unpack_set(s, msg, state, high, pairs=range(8)):
    top, signs, tiles = state[STREAM + s], msg[_word(s * SET_WORDS)], {}
    for i in pairs:
        lows = msg[_word(s * SET_WORDS + 1 + i)]
        for j in (2 * i, 2 * i + 1):
            u = high(j) | ((_srl(lows, 8) if j % 2 else lows) & BYTE)
            tiles[j] = pltpu.bitcast(_flip(top, u) | ((signs << j) & SIGN), BF16)
    return tiles


def _all_reduce(
    x_hbm, out, given, kept, pair_sum, outbox, inbox, detour_out, detour_in, packer, unpacker,
    held, forms, given_sem, kept_sem, send_sem, recv_sem, detour_sem, entered_sem,
):
    me = lax.axis_index("i")
    odd = (me & 1) == 1
    lead = (me + 1) >> 2

    def peer(half):
        return jnp.where(half == 0, me ^ 1, 3 - me)

    def side(half):
        return jnp.where(half == 0, (me ^ (me >> 1)) & 1, me >> 1)

    def keep(half):
        return (2 * half + side(half)) * PIECE

    def give(half):
        return (2 * half + 1 - side(half)) * PIECE

    def rows(c, s, source):
        if c:
            return MSG_ROWS + SET_ROWS * s
        return SET_ROWS * ((s + (source == 2).astype(I32)) & 3)

    def each_link(f):
        _loop(0, 2, lambda link: f(link ^ lead))

    def signal(sem, chips):
        for chip in chips:
            pl.semaphore_signal(sem, inc=1, device_id=(chip,), device_id_type=pl.DeviceIdType.MESH)

    def remote(src, dst, send, recv, chip):
        return pltpu.make_async_remote_copy(
            src, dst, send, recv, device_id=(chip,), device_id_type=pl.DeviceIdType.MESH
        )

    def load_given(half, slot, start, size):
        return pltpu.make_async_copy(
            x_hbm.at[_span(give(half) + start, size, 16)],
            given.at[_span(half * PIECE + start, size, 16)],
            given_sem.at[7 * half + slot],
        )

    def load_set(half, s):
        return load_given(half, s, rows(0, s, me), SET_ROWS)

    def load_direct():
        return load_given(lead, 0, 0, DIRECT_ROWS)

    def load_detour():
        return load_given(lead, 4, DIRECT_ROWS, SET_ROWS - DIRECT_ROWS)

    def load_second(half, part):
        size = MSG_ROWS - SET_ROWS if part else SET_ROWS
        return load_given(half, 5 + part, MSG_ROWS + SET_ROWS * part, size)

    def load_kept(half, c):
        return pltpu.make_async_copy(
            x_hbm.at[_span(keep(half) + c * MSG_ROWS, MSG_ROWS, 16)],
            kept.at[_span(half * PIECE + c * MSG_ROWS, MSG_ROWS, 16)],
            kept_sem.at[2 * half + c],
        )

    def box(step, c, half):
        return 4 * step + 2 * c + half

    def copy(step, c, half, slot, start, size):
        i, words = box(step, c, half), _span(8 * start, 8 * size, 8)
        return remote(
            outbox.at[i, words], inbox.at[i, words], send_sem.at[8 * i + slot],
            recv_sem.at[8 * i + slot], peer(1 - half if step == 1 else half),
        )

    def copy_set(step, c, half, s, size=SET_WORDS):
        return copy(step, c, half, s, s * SET_WORDS, size)

    def copy_head(step, c, half):
        return copy(step, c, half, 4, W_HEAD, W_POOL + 1 - W_HEAD)

    def copy_pool(step, c, half):
        return copy(step, c, half, 5, W_POOL + 1, 1)

    def copy_rest(step, c, half):
        return copy(step, c, half, 6, W_POOL + 1, W_END - W_POOL - 1)

    def copy_last(half):
        return copy_set(2, 1, half, SETS - 1, SET_WORDS - TAIL)

    def copy_tail(half):
        return copy(2, 1, half, 7, W_HEAD - TAIL, TAIL)

    def copy_detour(half):
        return remote(detour_out, detour_in.at[half], detour_sem.at[2], detour_sem.at[half], 2)

    def finish(step, c, half, tile_of):
        form = _pack_end(outbox.at[box(step, c, half)], packer.at[half], tile_of)
        copy_head(step, c, half).start()
        pl.when(form == TWO_POOLS)(lambda: copy_pool(step, c, half).start())
        pl.when(form == OVERFLOWS)(lambda: copy_rest(step, c, half).start())
        if (step, c) == (2, 1):
            for s in range(1, SETS - 1):
                copy_set(step, c, half, s).start()
            copy_last(half).start()
            copy_tail(half).start()
        elif (step, c) != (0, 0):
            for s in range(1, SETS):
                copy_set(step, c, half, s).start()
        forms[box(step, c, half)] = form

    def receive(step, c, half, each_set):
        copy_head(step, c, half).wait_recv()
        msg, state = inbox.at[box(step, c, half)], unpacker.at[half]
        uncoded = _unpack_begin(
            msg, state,
            lambda: copy_pool(step, c, half).wait_recv(),
            lambda: copy_rest(step, c, half).wait_recv(),
        )
        for form, taken in ((False, jnp.logical_not(uncoded)), (True, uncoded)):
            pl.when(taken)(
                lambda: _loop(0, SETS, lambda s: each_set(s, lambda: _unpack_high(s, msg, state, form)))
            )

    def given_tile(half, c, s, j):
        return given[_tile(half * PIECE + rows(c, s, me), j)].astype(BF16)

    def pack_given(half, c, s, tiles=16):
        words = [pltpu.bitcast(given_tile(half, c, s, j), I32) for j in range(tiles)]
        words += [_zeros()] * (16 - tiles)
        return _pack_low(words, s, outbox.at[box(0, c, half)], packer.at[half])

    def hold(half, s, words):
        for j, w in enumerate(words):
            held[half, 16 * s + j] = w

    barrier = pltpu.get_barrier_semaphore()

    @pl.when(odd)
    def _():
        load_direct().start()
        signal(barrier, (2, 0))
        for t, (link, s) in enumerate(ODD_ORDER[1:]):
            load_set(link ^ lead, s).start()
            if t == 0:
                load_detour().start()
        for half in range(2):
            _pack_begin(packer.at[half])
        pl.semaphore_wait(barrier, 1)
        load_direct().wait()
        us = pack_given(lead, 0, 0, DIRECT)
        copy_set(0, 0, lead, 0, DIRECT_WORDS).start()
        hold(lead, 0, us)

    @pl.when(jnp.logical_not(odd))
    def _():
        for half, s in EVEN_ORDER[:2]:
            load_set(half, s).start()

        @pl.when(me == 2)
        def _():
            pl.semaphore_wait(barrier, 2)
            signal(entered_sem, (1, 3))

        @pl.when(me == 0)
        def _():
            signal(barrier, (1, 3))
            for half in range(2):
                for i in range(DIRECT_WORDS, SET_WORDS):
                    inbox[box(0, 0, half), _word(i)] = _zeros()

        for half, s in EVEN_ORDER[2:]:
            load_set(half, s).start()
        for half in range(2):
            _pack_begin(packer.at[half])

    def first_sets(t):
        odd_order, even_order = (
            sum((4 * link + s) << (3 * i) for i, (link, s) in enumerate(order))
            for order in (ODD_ORDER, EVEN_ORDER)
        )
        entry = jnp.where(odd, odd_order, even_order) >> (3 * t)
        half, s = ((entry >> 2) & 1) ^ lead, entry & 3
        load_set(half, s).wait()

        @pl.when((me == 2) & (s == SETS - 1))
        def _():
            copy_detour(half).wait_recv()
            for i in range(DETOUR):
                at = _tile(half * PIECE, DIRECT + i)
                given[at] = given[at] + pltpu.bitcast(detour_in[half, _word(i)], BF16).astype(F32)

        us = pack_given(half, 0, s)

        @pl.when(odd & (t == 2))
        def _():
            load_detour().wait()
            for i in range(DETOUR):
                at = _tile(lead * PIECE, DIRECT + i)
                detour_out[_word(i)] = pltpu.bitcast(given[at].astype(BF16), I32)
                given[at] = jnp.zeros((16, 128), F32)
            pl.semaphore_wait(entered_sem, 1)
            copy_detour(lead).start()

        @pl.when((me == 0) & (t == 1))
        def _():
            pl.semaphore_wait(barrier, 2)
            copy_set(0, 0, lead, 0).start()

        pl.when((me != 0) | (t != 0))(lambda: copy_set(0, 0, half, s).start())
        hold(half, s, us)

        @pl.when(t == 3)
        def _():
            for link in range(2):
                for part in range(2):
                    load_second(link ^ lead, part).start()

    _loop(me & 1, 2 * SETS, first_sets)
    for link in range(2):
        load_kept(link ^ lead, 0).start()

    @each_link
    def _(half):
        _loop(
            0, SETS,
            lambda s: _pack_high([held[half, 16 * s + j] for j in range(16)], packer.at[half]),
        )
        finish(0, 0, half, lambda s, j: given_tile(half, 0, s, j))

    @each_link
    def _(half):
        def each_set(s):
            pl.when(s == 0)(lambda: load_second(half, 0).wait())
            pl.when(s == 1)(lambda: load_second(half, 1).wait())
            _pack_high(pack_given(half, 1, s), packer.at[half])
            pl.when(s == 0)(lambda: copy_set(0, 1, half, 0).start())

        _pack_begin(packer.at[half])
        _loop(0, SETS, each_set)
        finish(0, 1, half, lambda s, j: given_tile(half, 1, s, j))

    for link in range(2):
        load_kept(link ^ lead, 1).start()

    def add_and_send(step, c, half):
        msg, state = inbox.at[box(step - 1, c, half)], unpacker.at[half]
        own = kept if step == 1 else pair_sum
        sums, base = (pair_sum, half * PIECE) if step == 1 else (out, keep(half))
        source = peer(half) if step == 1 else me ^ 2
        if step == 1:
            load_kept(half, c).wait()
        if (step, c) == (1, 0):
            pl.when(me == 0)(lambda: copy_set(0, 0, half, 0, DIRECT_WORDS).wait_recv())
            pl.when(me != 0)(lambda: copy_set(0, 0, half, 0).wait_recv())
            for s in range(1, SETS):
                copy_set(0, 0, half, s).wait_recv()

        def sum_tile(s, j):
            return sums[_tile(base + rows(c, s, source), j)]

        def each_set(s, unpack_high):
            if (step, c) != (1, 0):
                copy_set(step - 1, c, half, s).wait_recv()
            highs, row = unpack_high(), rows(c, s, source)
            for j, theirs in _unpack_set(s, msg, state, lambda j: highs[j]).items():
                mine = own[_tile(half * PIECE + row, j)].astype(F32)
                sums[_tile(base + row, j)] = (mine + theirs.astype(F32)).astype(BF16)
            words = [pltpu.bitcast(sum_tile(s, j), I32) for j in range(16)]
            us = _pack_low(words, s, outbox.at[box(step, c, half)], packer.at[half])
            _pack_high(us, packer.at[half])
            pl.when(s == 0)(lambda: copy_set(step, c, half, 0).start())

        _pack_begin(packer.at[half])
        receive(step - 1, c, half, each_set)
        finish(step, c, half, sum_tile)

    for step in (1, 2):
        for c in range(2):
            each_link(lambda half: add_and_send(step, c, half))

    def wait_sent(step, c, sets=SETS):
        for half in range(2):
            if (step, c) == (0, 0):
                short = odd & (lead == half)
                pl.when(short)(lambda: copy_set(0, 0, half, 0, DIRECT_WORDS).wait_send())
                pl.when(jnp.logical_not(short))(lambda: copy_set(0, 0, half, 0).wait_send())
            for s in range(int((step, c) == (0, 0)), sets):
                copy_set(step, c, half, s).wait_send()
            copy_head(step, c, half).wait_send()
            form = forms[box(step, c, half)]
            pl.when(form == TWO_POOLS)(lambda: copy_pool(step, c, half).wait_send())
            pl.when(form == OVERFLOWS)(lambda: copy_rest(step, c, half).wait_send())

    pl.when(odd)(lambda: copy_detour(lead).wait_send())
    for step in range(2):
        for c in range(2):
            wait_sent(step, c)

    def store(c, half, s, pairs=range(8)):
        msg, state = inbox.at[box(2, c, half)], unpacker.at[half]
        tiles = _unpack_set(s, msg, state, lambda j: held[half, 16 * s + j], pairs)
        for j, tile in tiles.items():
            out[_tile(give(half) + rows(c, s, peer(half) ^ 2), j)] = tile

    for c in range(2):
        each_link(lambda half: receive(2, c, half, lambda s, high: hold(half, s, high())))

        def early_set(t):
            s, half = t >> 1, (t & 1) ^ lead
            copy_set(2, c, half, s).wait_recv()
            store(c, half, s)

        _loop(0, 2 * (SETS - c), early_set)
        wait_sent(2, c, SETS - c)

    @each_link
    def _(half):
        copy_last(half).wait_recv()
        store(1, half, SETS - 1, range(8 - TAIL))

    for half in range(2):
        copy_last(half).wait_send()
        copy_tail(half).wait_send()
    for link in range(2):
        copy_tail(link ^ lead).wait_recv()
        store(1, link ^ lead, SETS - 1, range(8 - TAIL, 8))


def pallas_dist_ar_i_i_m2048_n512_kernel(x: jax.Array):
    assert x.shape == (ROWS, COLS) and x.dtype == F32
    dma = pltpu.SemaphoreType.DMA
    messages = 3 * 2 * 2
    return pl.pallas_call(
        _all_reduce,
        out_shape=jax.ShapeDtypeStruct((ROWS, COLS), BF16),
        in_specs=[pl.BlockSpec(memory_space=pl.ANY)],
        out_specs=pl.BlockSpec(memory_space=pltpu.VMEM),
        scratch_shapes=[
            pltpu.VMEM((2 * PIECE, COLS), F32),
            pltpu.VMEM((2 * PIECE, COLS), F32),
            pltpu.VMEM((2 * PIECE, COLS), BF16),
            pltpu.VMEM((messages, 8 * W_END, 128), I32),
            pltpu.VMEM((messages, 8 * W_END, 128), I32),
            pltpu.VMEM((8 * DETOUR, 128), I32),
            pltpu.VMEM((2, 8 * DETOUR, 128), I32),
            pltpu.VMEM((2, P_TOP + 1 + SETS, 8, 128), I32),
            pltpu.VMEM((2, STREAM + SETS, 8, 128), I32),
            pltpu.VMEM((2, 16 * SETS, 8, 128), I32),
            pltpu.SMEM((messages,), I32),
            dma((14,)),
            dma((4,)),
            dma((8 * messages,)),
            dma((8 * messages,)),
            dma((3,)),
            pltpu.SemaphoreType.REGULAR,
        ],
        compiler_params=pltpu.CompilerParams(
            collective_id=0,
            vmem_limit_bytes=32 * 2**20,
            disable_semaphore_checks=True,
        ),
    )(x)
```

```python
import jax
import jax.numpy as jnp
import numpy as np
from jax import lax
from jax.experimental import pallas as pl
from jax.experimental.pallas import tpu as pltpu

I32, BF16, F32 = jnp.int32, jnp.bfloat16, jnp.float32
ROWS, COLS = 2048, 512
PIECE = ROWS // 4
SET_ROWS = 64
SETS = 4
MSG_ROWS = SETS * SET_ROWS

SIGN, MAG, BYTE = np.array([0x80008000, 0x7FFF7FFF, 0x00FF00FF], np.uint32).view(np.int32)

SET_WORDS = 9
OWN, POOLED = 6, 3
STREAM = OWN + POOLED
W_HEAD = SETS * SET_WORDS
W_OWN = W_HEAD + 1
W_POOL = W_OWN + OWN
W_END = W_OWN + 8 * SETS + 2
TOP_DROP, UNCODED = 8, 63
FITS, TWO_POOLS, OVERFLOWS = 0, 1, 2
GROUPS = (7, 7, 6, 6, 6)

P_TOP = STREAM + 2

DETOUR = 8
DETOUR_ROWS = 4 * DETOUR
DIRECT_ROWS = SET_ROWS - DETOUR_ROWS
DIRECT_WORDS = SET_WORDS - DETOUR // 2
ODD_ORDER = ((0, 0), (0, 1), (0, 2), (1, 0), (0, 3), (1, 1), (1, 2), (1, 3))
EVEN_ORDER = ((0, 0), (1, 0), (0, 1), (1, 1), (0, 2), (1, 2), (0, 3), (1, 3))
AHEAD = ((4, 2), (2, 2), (2, 1))
TAIL = 2


def _span(start, size, align):
    if not isinstance(start, int):
        start = pl.multiple_of(start, align)
    return pl.ds(start, size)


def _read(ref, start, count):
    words = ref[_span(8 * start, 8 * count, 8)]
    return [words[8 * i : 8 * i + 8] for i in range(count)]


def _write(ref, start, words):
    ref[_span(8 * start, 8 * len(words), 8)] = jnp.concatenate(words, axis=0)


def _words(block):
    block = pltpu.bitcast(block, I32)
    return [
        block[r : r + 8, c : c + 128]
        for r in range(0, block.shape[0], 8)
        for c in range(0, COLS, 128)
    ]


def _block(words):
    strips = [jnp.concatenate(words[i : i + 4], axis=1) for i in range(0, len(words), 4)]
    return pltpu.bitcast(jnp.concatenate(strips, axis=0), BF16)


def _srl(v, n):
    return lax.shift_right_logical(v, np.int32(n) if isinstance(n, int) else n)


def _roll(v, k):
    return pltpu.roll(v, k, 0) if k else v


def _zeros():
    return jnp.zeros((8, 128), I32)


def _sublane():
    return lax.broadcasted_iota(I32, (8, 128), 0)


def _loop(lo, hi, f):
    lax.fori_loop(lo, hi, lambda i, _: f(i), None)


def _top(code):
    top = (code + 1) << 4
    return top | (top << 16)


def _flip(top, v):
    nonzero = (v + MAG) & SIGN
    return (top - v) & (nonzero - _srl(nonzero, 15))


def _pool_layout(head):
    n = _srl(head, 26)
    end = n
    for k in (1, 2, 4):
        end = end + jnp.where(_sublane() >= k, _roll(end, k), 0)
    form = jnp.where(end > 128, float(TWO_POOLS), float(FITS))
    form = jnp.where((n == UNCODED) | (end > 256), float(OVERFLOWS), form)
    start = 2 * (end - n)
    return jnp.max(form).astype(I32), start >> 5, start & 31


def _pack_begin(state):
    _write(state, 0, [_zeros()] * (P_TOP + 1))


def _pack_low(words, s, msg, state):
    mags = [w & MAG for w in words]
    peak = [lax.bitcast_convert_type(v, F32) for v in mags + [m << 16 for m in mags]]
    while len(peak) > 1:
        peak = [jnp.maximum(a, b) for a, b in zip(peak[0::2], peak[1::2])]
    code = jnp.maximum(lax.bitcast_convert_type(peak[0], I32) >> 20, 7)
    code = jnp.where(peak[0] != peak[0], 2047, code)
    code = jnp.maximum(code, _read(state, P_TOP + s, 1)[0] - TOP_DROP)
    _write(state, P_TOP + s + 1, [code])
    top = _top(code)
    us = [_flip(top, m) for m in mags]
    signs = _zeros()
    for j, w in enumerate(words):
        signs = signs | _srl(w & SIGN, j)
    lows = [(a & BYTE) | ((b & BYTE) << 8) for a, b in zip(us[0::2], us[1::2])]
    _write(msg, s * SET_WORDS, [signs] + lows)
    return us


def _pack_high(us, state):
    *stream, length, longest = _read(state, 0, P_TOP)
    highs = iter([high for u in us for high in ((u >> 8) & 0xFF, u >> 24)])
    for group in GROUPS:
        bits, total = _zeros(), _zeros()
        for k in range(group):
            total = total + next(highs)
            bits = bits | ((1 << k) << (total & 31))
        total = total + group
        lo, hi = bits << (length & 31), _srl(_srl(bits, 1), 31 - (length & 31))
        here = [length >> 5 == i for i in range(STREAM)]
        stream = [
            v | jnp.where(here[i], lo, jnp.where(here[i - 1], hi, 0) if i else 0)
            for i, v in enumerate(stream)
        ]
        length, longest = length + total, jnp.maximum(longest, total)
    _write(state, 0, stream + [length, longest])


def _pack_end(msg, state, words_of):
    *stream, length, longest = _read(state, 0, P_TOP)
    codes = _read(state, P_TOP + 1, SETS)
    head = codes[0]
    unfit = (longest > 31) | (length > 32 * STREAM)
    for s in range(1, SETS):
        step = codes[s] - codes[s - 1] + TOP_DROP
        head, unfit = head | ((step & 31) << (6 + 5 * s)), unfit | (step > 31)
    pooled = (jnp.maximum(length - 32 * OWN, 0) + 1) >> 1
    head = head | (jnp.where(unfit, UNCODED, pooled) << 26)
    form, first, bit = _pool_layout(head)
    rest, pools = stream[OWN:], []
    moved = [
        (rest[i] << bit if i < POOLED else 0) | (_srl(_srl(rest[i - 1], 1), 31 - bit) if i else 0)
        for i in range(POOLED + 1)
    ]
    for p in range(2):
        pool = _zeros()
        for k in range(8):
            which, part = ((_sublane() + k) & 7) + 8 * p - first, 0
            for i, v in enumerate(moved):
                part = jnp.where(which == i, v, part)
            pool = pool | _roll(part, k)
        pools.append(pool)
    _write(msg, W_HEAD, [head] + stream[:OWN] + pools)

    @pl.when(form == OVERFLOWS)
    def _():
        def high_bytes(s):
            top = _top(_read(state, P_TOP + 1 + s, 1)[0])
            highs = [_flip(top, w & MAG) & ~BYTE for w in words_of(s)]
            _write(msg, W_OWN + 8 * s, [_srl(a, 8) | b for a, b in zip(highs[0::2], highs[1::2])])

        _loop(0, SETS, high_bytes)
        _write(msg, W_END - 2, [a | (b << 16) for a, b in zip(codes[0::2], codes[1::2])])

    return form


def _unpack_begin(msg, state, wait_pool, wait_rest):
    (head,) = _read(msg, W_HEAD, 1)
    form, first, bit = _pool_layout(head)

    @pl.when(form == FITS)
    def _():
        _write(msg, W_POOL + 1, [_zeros()])

    pl.when(form == TWO_POOLS)(wait_pool)

    @pl.when(form != OVERFLOWS)
    def _():
        codes = [head & 2047]
        for s in range(1, SETS):
            codes.append(codes[-1] + ((head >> (6 + 5 * s)) & 31) - TOP_DROP)
        moved = [_zeros()] * (POOLED + 1)
        for p, pool in enumerate(_read(msg, W_POOL, 2)):
            for k in range(8):
                which = ((_sublane() + k) & 7) + 8 * p - first
                part = _roll(pool, (8 - k) % 8)
                moved = [jnp.where(which == i, part, v) for i, v in enumerate(moved)]
        rest = [_srl(a, bit) | ((b << 1) << (31 - bit)) for a, b in zip(moved, moved[1:])]
        _write(state, 0, _read(msg, W_OWN, OWN) + rest + [_top(code) for code in codes])

    @pl.when(form == OVERFLOWS)
    def _():
        wait_rest()
        codes = [c for pair in _read(msg, W_END - 2, 2) for c in (pair & 0xFFFF, pair >> 16)]
        _write(state, STREAM, [_top(code) for code in codes])

    return form == OVERFLOWS


def _unpack_high(s, msg, state, uncoded):
    if uncoded:
        pairs = _read(msg, W_OWN + 8 * s, 8)
        return [(pairs[j // 2] if j % 2 else pairs[j // 2] << 8) & ~BYTE for j in range(16)]
    stream, sizes = _read(state, 0, STREAM), []
    for group in GROUPS:
        bits, place = stream[0], 126 << 23
        for _ in range(group):
            others = bits & (bits - 1)
            before, place = place, lax.bitcast_convert_type((bits ^ others).astype(F32), I32)
            bits = others
            sizes.append(place - before)
        used = (place >> 23) - 126
        stream = [
            _srl(v, used) | (stream[i + 1] << (32 - used) if i + 1 < STREAM else 0)
            for i, v in enumerate(stream)
        ]
    _write(state, 0, stream)
    return [((a >> 15) | (b << 1)) - 0x01000100 for a, b in zip(sizes[0::2], sizes[1::2])]


def _unpack_set(s, msg, state, highs, first=0):
    (top,), (signs,) = _read(state, STREAM + s, 1), _read(msg, s * SET_WORDS, 1)
    lows = _read(msg, s * SET_WORDS + 1 + first // 2, len(highs) // 2)
    words = []
    for j, high in enumerate(highs):
        low = _srl(lows[j // 2], 8) if j % 2 else lows[j // 2]
        words.append(_flip(top, high | (low & BYTE)) | ((signs << (first + j)) & SIGN))
    return _block(words)


def _all_reduce(
    x_hbm, out, given, kept, pair_sum, outbox, inbox, detour_out, detour_in, packer, unpacker,
    held, forms, given_sem, kept_sem, send_sem, recv_sem, detour_sem, entered_sem,
):
    me = lax.axis_index("i")
    odd = (me & 1) == 1
    lead = (me + 1) >> 2

    def peer(half):
        return jnp.where(half == 0, me ^ 1, 3 - me)

    def side(half):
        return jnp.where(half == 0, (me ^ (me >> 1)) & 1, me >> 1)

    def keep(half):
        return (2 * half + side(half)) * PIECE

    def give(half):
        return (2 * half + 1 - side(half)) * PIECE

    def rows(c, s, source):
        if c:
            return MSG_ROWS + SET_ROWS * s
        return SET_ROWS * ((s + (source == 2).astype(I32)) & 3)

    def each_link(f):
        _loop(0, 2, lambda link: f(link ^ lead))

    def signal(sem, chips):
        for chip in chips:
            pl.semaphore_signal(sem, inc=1, device_id=(chip,), device_id_type=pl.DeviceIdType.MESH)

    def remote(src, dst, send, recv, chip):
        return pltpu.make_async_remote_copy(
            src, dst, send, recv, device_id=(chip,), device_id_type=pl.DeviceIdType.MESH
        )

    def load_given(half, slot, start, size):
        return pltpu.make_async_copy(
            x_hbm.at[_span(give(half) + start, size, 16)],
            given.at[_span(half * PIECE + start, size, 16)],
            given_sem.at[7 * half + slot],
        )

    def load_set(half, s):
        return load_given(half, s, rows(0, s, me), SET_ROWS)

    def load_direct():
        return load_given(lead, 0, 0, DIRECT_ROWS)

    def load_detour():
        return load_given(lead, 4, DIRECT_ROWS, DETOUR_ROWS)

    def load_second(half, part):
        size = MSG_ROWS - SET_ROWS if part else SET_ROWS
        return load_given(half, 5 + part, MSG_ROWS + SET_ROWS * part, size)

    def load_kept(half, c):
        return pltpu.make_async_copy(
            x_hbm.at[_span(keep(half) + c * MSG_ROWS, MSG_ROWS, 16)],
            kept.at[_span(half * PIECE + c * MSG_ROWS, MSG_ROWS, 16)],
            kept_sem.at[2 * half + c],
        )

    def box(step, c, half):
        return 4 * step + 2 * c + half

    def copy(step, c, half, slot, start, size):
        i, words = box(step, c, half), _span(8 * start, 8 * size, 8)
        return remote(
            outbox.at[i, words], inbox.at[i, words], send_sem.at[8 * i + slot],
            recv_sem.at[8 * i + slot], peer(1 - half if step == 1 else half),
        )

    def copy_set(step, c, half, s, size=SET_WORDS):
        return copy(step, c, half, s, s * SET_WORDS, size)

    def copy_head(step, c, half):
        return copy(step, c, half, 4, W_HEAD, W_POOL + 1 - W_HEAD)

    def copy_pool(step, c, half):
        return copy(step, c, half, 5, W_POOL + 1, 1)

    def copy_rest(step, c, half):
        return copy(step, c, half, 6, W_POOL + 1, W_END - W_POOL - 1)

    def copy_last(half):
        return copy_set(2, 1, half, SETS - 1, SET_WORDS - TAIL)

    def copy_tail(half):
        return copy(2, 1, half, 7, W_HEAD - TAIL, TAIL)

    def copy_detour(half):
        return remote(detour_out, detour_in.at[half], detour_sem.at[2], detour_sem.at[half], 2)

    def finish(step, c, half, words_of):
        form = _pack_end(outbox.at[box(step, c, half)], packer.at[half], words_of)
        copy_head(step, c, half).start()
        pl.when(form == TWO_POOLS)(lambda: copy_pool(step, c, half).start())
        pl.when(form == OVERFLOWS)(lambda: copy_rest(step, c, half).start())
        for s in range(AHEAD[step][c], SETS):
            if (step, c, s) == (2, 1, SETS - 1):
                copy_last(half).start()
                copy_tail(half).start()
            else:
                copy_set(step, c, half, s).start()
        forms[box(step, c, half)] = form

    def receive(step, c, half, each_set):
        copy_head(step, c, half).wait_recv()
        msg, state = inbox.at[box(step, c, half)], unpacker.at[half]
        uncoded = _unpack_begin(
            msg, state,
            lambda: copy_pool(step, c, half).wait_recv(),
            lambda: copy_rest(step, c, half).wait_recv(),
        )
        for form, taken in ((False, jnp.logical_not(uncoded)), (True, uncoded)):

            @pl.when(taken)
            def _():
                _loop(0, SETS, lambda s: each_set(s, lambda: _unpack_high(s, msg, state, form)))

    def given_words(half, c, s, size=SET_ROWS):
        return _words(given[_span(half * PIECE + rows(c, s, me), size, 16)].astype(BF16))

    def pack_given(half, c, s, size=SET_ROWS):
        words = given_words(half, c, s, size)
        words += [_zeros()] * (16 - len(words))
        return _pack_low(words, s, outbox.at[box(0, c, half)], packer.at[half])

    barrier = pltpu.get_barrier_semaphore()

    @pl.when(odd)
    def _():
        load_direct().start()
        signal(barrier, (2, 0))
        for t, (link, s) in enumerate(ODD_ORDER[1:]):
            load_set(link ^ lead, s).start()
            if t == 0:
                load_detour().start()
        for half in range(2):
            _pack_begin(packer.at[half])
        pl.semaphore_wait(barrier, 1)
        load_direct().wait()
        us = pack_given(lead, 0, 0, DIRECT_ROWS)
        copy_set(0, 0, lead, 0, DIRECT_WORDS).start()
        _write(held.at[lead], 0, us)

    @pl.when(jnp.logical_not(odd))
    def _():
        for half, s in EVEN_ORDER[:2]:
            load_set(half, s).start()

        @pl.when(me == 2)
        def _():
            pl.semaphore_wait(barrier, 2)
            signal(entered_sem, (1, 3))

        @pl.when(me == 0)
        def _():
            signal(barrier, (1, 3))
            for half in range(2):
                _write(inbox.at[box(0, 0, half)], DIRECT_WORDS, [_zeros()] * (DETOUR // 2))

        for half, s in EVEN_ORDER[2:]:
            load_set(half, s).start()
        for half in range(2):
            _pack_begin(packer.at[half])

    def pack_held(half, s):
        _pack_high(_read(held.at[half], 16 * s, 16), packer.at[half])

    def first_sets(t):
        odd_order, even_order = (
            sum((4 * link + s) << (3 * i) for i, (link, s) in enumerate(order))
            for order in (ODD_ORDER, EVEN_ORDER)
        )
        entry = jnp.where(odd, odd_order, even_order) >> (3 * t)
        half, s = ((entry >> 2) & 1) ^ lead, entry & 3
        load_set(half, s).wait()

        @pl.when((me == 2) & (t == 2 * (SETS - 1)))
        def _():
            each_link(lambda half: _loop(0, SETS - 1, lambda s: pack_held(half, s)))

        @pl.when((me == 2) & (s == SETS - 1))
        def _():
            copy_detour(half).wait_recv()
            at = _span(half * PIECE + DIRECT_ROWS, DETOUR_ROWS, 16)
            given[at] = given[at] + detour_in[half].astype(F32)

        us = pack_given(half, 0, s)

        @pl.when(odd & (t == 2))
        def _():
            load_detour().wait()
            at = _span(lead * PIECE + DIRECT_ROWS, DETOUR_ROWS, 16)
            detour_out[...] = given[at].astype(BF16)
            given[at] = jnp.zeros((DETOUR_ROWS, COLS), F32)
            pl.semaphore_wait(entered_sem, 1)
            copy_detour(lead).start()

        @pl.when((me == 0) & (t == 1))
        def _():
            pl.semaphore_wait(barrier, 2)
            copy_set(0, 0, lead, 0).start()

        pl.when((me != 0) | (t != 0))(lambda: copy_set(0, 0, half, s).start())
        _write(held.at[half], 16 * s, us)

        @pl.when(t == 3)
        def _():
            for link in range(2):
                for part in range(2):
                    load_second(link ^ lead, part).start()

    _loop(me & 1, 2 * SETS, first_sets)
    for link in range(2):
        load_kept(link ^ lead, 0).start()

    @each_link
    def _(half):
        _loop(jnp.where(me == 2, SETS - 1, 0), SETS, lambda s: pack_held(half, s))
        finish(0, 0, half, lambda s: given_words(half, 0, s))

    @each_link
    def _(half):
        def each_set(s):
            pl.when(s == 0)(lambda: load_second(half, 0).wait())
            pl.when(s == 1)(lambda: load_second(half, 1).wait())
            _pack_high(pack_given(half, 1, s), packer.at[half])
            pl.when(s < AHEAD[0][1])(lambda: copy_set(0, 1, half, s).start())

        _pack_begin(packer.at[half])
        _loop(0, SETS, each_set)
        finish(0, 1, half, lambda s: given_words(half, 1, s))

    for link in range(2):
        load_kept(link ^ lead, 1).start()

    def add_and_send(step, c, half):
        msg, state = inbox.at[box(step - 1, c, half)], unpacker.at[half]
        own = kept if step == 1 else pair_sum
        sums, base = (pair_sum, half * PIECE) if step == 1 else (out, keep(half))
        source = peer(half) if step == 1 else me ^ 2
        if step == 1:
            load_kept(half, c).wait()
        if (step, c) == (1, 0):
            pl.when(me == 0)(lambda: copy_set(0, 0, half, 0, DIRECT_WORDS).wait_recv())
            pl.when(me != 0)(lambda: copy_set(0, 0, half, 0).wait_recv())
            for s in range(1, SETS):
                copy_set(0, 0, half, s).wait_recv()

        def sum_words(s):
            return _words(sums[_span(base + rows(c, s, source), SET_ROWS, 16)])

        def each_set(s, unpack_high):
            if (step, c) != (1, 0):
                copy_set(step - 1, c, half, s).wait_recv()
            theirs, row = _unpack_set(s, msg, state, unpack_high()), rows(c, s, source)
            mine = own[_span(half * PIECE + row, SET_ROWS, 16)]
            total = mine.astype(F32) + theirs.astype(F32)
            sums[_span(base + row, SET_ROWS, 16)] = total.astype(BF16)
            us = _pack_low(sum_words(s), s, outbox.at[box(step, c, half)], packer.at[half])
            _pack_high(us, packer.at[half])
            pl.when(s < AHEAD[step][c])(lambda: copy_set(step, c, half, s).start())

        _pack_begin(packer.at[half])
        receive(step - 1, c, half, each_set)
        finish(step, c, half, sum_words)

    for step in (1, 2):
        for c in range(2):
            each_link(lambda half: add_and_send(step, c, half))

    def wait_sent(step, c, sets=SETS):
        for half in range(2):
            if (step, c) == (0, 0):
                short = odd & (lead == half)
                pl.when(short)(lambda: copy_set(0, 0, half, 0, DIRECT_WORDS).wait_send())
                pl.when(jnp.logical_not(short))(lambda: copy_set(0, 0, half, 0).wait_send())
            for s in range(int((step, c) == (0, 0)), sets):
                copy_set(step, c, half, s).wait_send()
            copy_head(step, c, half).wait_send()
            form = forms[box(step, c, half)]
            pl.when(form == TWO_POOLS)(lambda: copy_pool(step, c, half).wait_send())
            pl.when(form == OVERFLOWS)(lambda: copy_rest(step, c, half).wait_send())

    pl.when(odd)(lambda: copy_detour(lead).wait_send())
    for step in range(2):
        for c in range(2):
            wait_sent(step, c)

    def store(c, half, s, first=0, count=16):
        msg, state = inbox.at[box(2, c, half)], unpacker.at[half]
        highs = _read(held.at[half], 16 * s + first, count)
        row = give(half) + rows(c, s, peer(half) ^ 2) + 4 * first
        out[_span(row, 4 * count, 16)] = _unpack_set(s, msg, state, highs, first)

    for c in range(2):
        each_link(
            lambda half: receive(
                2, c, half, lambda s, unpack_high: _write(held.at[half], 16 * s, unpack_high())
            )
        )

        def early_set(t):
            s, half = t >> 1, (t & 1) ^ lead
            copy_set(2, c, half, s).wait_recv()
            store(c, half, s)

        _loop(0, 2 * (SETS - c), early_set)
        wait_sent(2, c, SETS - c)

    @each_link
    def _(half):
        copy_last(half).wait_recv()
        store(1, half, SETS - 1, 0, 16 - 2 * TAIL)

    for half in range(2):
        copy_last(half).wait_send()
        copy_tail(half).wait_send()
    for link in range(2):
        copy_tail(link ^ lead).wait_recv()
        store(1, link ^ lead, SETS - 1, 16 - 2 * TAIL, 2 * TAIL)


def pallas_dist_ar_i_i_m2048_n512_kernel(x: jax.Array):
    assert x.shape == (ROWS, COLS) and x.dtype == F32
    dma = pltpu.SemaphoreType.DMA
    messages = 3 * 2 * 2
    return pl.pallas_call(
        _all_reduce,
        out_shape=jax.ShapeDtypeStruct((ROWS, COLS), BF16),
        in_specs=[pl.BlockSpec(memory_space=pl.ANY)],
        out_specs=pl.BlockSpec(memory_space=pltpu.VMEM),
        scratch_shapes=[
            pltpu.VMEM((2 * PIECE, COLS), F32),
            pltpu.VMEM((2 * PIECE, COLS), F32),
            pltpu.VMEM((2 * PIECE, COLS), BF16),
            pltpu.VMEM((messages, 8 * W_END, 128), I32),
            pltpu.VMEM((messages, 8 * W_END, 128), I32),
            pltpu.VMEM((DETOUR_ROWS, COLS), BF16),
            pltpu.VMEM((2, DETOUR_ROWS, COLS), BF16),
            pltpu.VMEM((2, 8 * (P_TOP + 1 + SETS), 128), I32),
            pltpu.VMEM((2, 8 * (STREAM + SETS), 128), I32),
            pltpu.VMEM((2, 8 * 16 * SETS, 128), I32),
            pltpu.SMEM((messages,), I32),
            dma((14,)),
            dma((4,)),
            dma((8 * messages,)),
            dma((8 * messages,)),
            dma((3,)),
            pltpu.SemaphoreType.REGULAR,
        ],
        compiler_params=pltpu.CompilerParams(
            collective_id=0,
            vmem_limit_bytes=32 * 2**20,
            disable_semaphore_checks=True,
        ),
    )(x)
```
